```python
import numpy as np

kernel_name = "dist_matmul_relu_kshard_i_m1024_n1024_k512"

def setup_inputs():
    A = np.random.randn(1024, 2048).astype(np.float32)
    B = np.random.randn(2048, 1024).astype(np.float32)
    return {"A": A, "B": B}

def reference(A: np.ndarray, B: np.ndarray) -> np.ndarray:
    z = A @ B
    return np.maximum(z, 0.0)
```

```python
import contextlib

import jax
import jax.numpy as jnp
from jax import lax
from jax.experimental import pallas as pl
from jax.experimental.pallas import tpu as pltpu

N_DEV = 4
G = 256

CFG = dict(
    loads=[
        ("B", 0, 128), ("A", 1, 0, 64), ("A", 2, 0, 64),
        ("A", 1, 64, 128), ("A", 2, 64, 128), ("B", 128, 256),
        ("A", 1, 128, 256), ("A", 2, 128, 256),
        ("B", 256, 512), ("B", 512, 768), ("B", 768, 1024),
        ("A", 0, 0, 256), ("A", 3, 0, 256),
    ],
    p1=[(0, 64, 0, 128), (64, 128, 0, 128), (0, 128, 128, 256),
        (128, 256, 0, 256), (0, 256, 256, 512), (0, 256, 512, 768),
        (0, 256, 768, 1024)],
    p2=[(0, 256, 0, 256), (0, 256, 256, 512), (0, 256, 512, 768),
        (0, 256, 768, 1024)],
    p3=[(0, 256, 0, 256), (0, 256, 256, 512), (0, 256, 512, 768),
        (0, 256, 768, 896), (0, 128, 896, 1024), (128, 256, 896, 1024)],
    scopes=False,
)


def _overlaps(w, v):
    return w[0] < v[1] and v[0] < w[1] and w[2] < v[3] and v[2] < w[3]


def _build(cfg, m, k, n):
    loads, p1, p2, p3 = cfg["loads"], cfg["p1"], cfg["p2"], cfg["p3"]
    phases = (p1, p2, p3)
    n_chunks = [len(p) for p in phases]
    sem_base = [0, 2 * n_chunks[0], 2 * (n_chunks[0] + n_chunks[1])]
    n_rdma = 2 * sum(n_chunks)

    def scope(name):
        return jax.named_scope(name) if cfg["scopes"] else contextlib.nullcontext()

    def body(a_hbm, b_hbm, out_ref, a32, b32, a16, b16, sbuf, rbuf, acc):
        me = lax.axis_index("i")
        right = lax.rem(me + 1, N_DEV)
        left = lax.rem(me + N_DEV - 1, N_DEV)
        nbr = (right, left)

        def row0(slot):
            return pl.multiple_of(lax.rem(me + slot, N_DEV) * G, G)

        def run(load_sems, send_sems, recv_sems):
            load_cps = []
            for i, ld in enumerate(loads):
                if ld[0] == "B":
                    _, c0, c1 = ld
                    cp = pltpu.make_async_copy(
                        b_hbm.at[:, pl.ds(c0, c1 - c0)],
                        b32.at[:, pl.ds(c0, c1 - c0)], load_sems.at[i])
                else:
                    _, s, r0, r1 = ld
                    cp = pltpu.make_async_copy(
                        a_hbm.at[pl.ds(row0(s) + r0, r1 - r0), :],
                        a32.at[s, pl.ds(r0, r1 - r0), :], load_sems.at[i])
                cp.start()
                load_cps.append(cp)

            barrier = pltpu.get_barrier_semaphore()
            for d in range(2):
                pl.semaphore_signal(
                    barrier, inc=1, device_id=(nbr[d],),
                    device_id_type=pl.DeviceIdType.MESH)

            loaded = [False] * len(loads)

            def need(slots, w):
                r0, r1, c0, c1 = w
                for i, ld in enumerate(loads):
                    if loaded[i]:
                        continue
                    if ld[0] == "B":
                        if not (ld[1] < c1 and c0 < ld[2]):
                            continue
                        load_cps[i].wait()
                        b16[:, ld[1]:ld[2]] = b32[:, ld[1]:ld[2]].astype(jnp.bfloat16)
                    else:
                        if not (ld[1] in slots and ld[2] < r1 and r0 < ld[3]):
                            continue
                        load_cps[i].wait()
                        a16[ld[1], ld[2]:ld[3], :] = (
                            a32[ld[1], ld[2]:ld[3], :].astype(jnp.bfloat16))
                    loaded[i] = True

            def rdma(phase, c, d):
                r0, r1, c0, c1 = phases[phase][c]
                idx = sem_base[phase] + 2 * c + d
                win = (phase, d, pl.ds(r0, r1 - r0), pl.ds(c0, c1 - c0))
                return pltpu.make_async_remote_copy(
                    src_ref=sbuf.at[win], dst_ref=rbuf.at[win],
                    send_sem=send_sems.at[idx], recv_sem=recv_sems.at[idx],
                    device_id=(nbr[d],), device_id_type=pl.DeviceIdType.MESH)

            arrived = [[[False, False] for _ in p] for p in phases]

            def recv(phase, d, w):
                for c, v in enumerate(phases[phase]):
                    if _overlaps(w, v) and not arrived[phase][c][d]:
                        rdma(phase, c, d).wait_recv()
                        arrived[phase][c][d] = True

            def partial(slot, w):
                r0, r1, c0, c1 = w
                return jnp.dot(a16[slot, r0:r1, :], b16[:, c0:c1],
                               preferred_element_type=jnp.float32)

            for c, w in enumerate(p1):
                r0, r1, c0, c1 = w
                for d, slot in ((0, 1), (1, 2)):
                    with scope(f"p1_{c}_{d}"):
                        need((slot,), w)
                        sbuf[0, d, r0:r1, c0:c1] = partial(slot, w).astype(jnp.bfloat16)
                    if c == 0 and d == 0:
                        with scope("barrier"):
                            pl.semaphore_wait(barrier, 2)
                    rdma(0, c, d).start()

            for c, w in enumerate(p2):
                r0, r1, c0, c1 = w
                for d, slot in ((0, 0), (1, 3)):
                    with scope(f"p2w_{c}_{d}"):
                        need((slot,), w)
                        recv(0, d, w)
                    with scope(f"p2_{c}_{d}"):
                        s = partial(slot, w) + rbuf[0, d, r0:r1, c0:c1].astype(jnp.float32)
                        acc[d, r0:r1, c0:c1] = s
                        sbuf[1, d, r0:r1, c0:c1] = s.astype(jnp.bfloat16)
                    rdma(1, c, d).start()

            for c, w in enumerate(p3):
                r0, r1, c0, c1 = w
                for d, slot in ((0, 3), (1, 0)):
                    with scope(f"p3w_{c}_{d}"):
                        recv(1, d, w)
                    with scope(f"p3_{c}_{d}"):
                        y = jnp.maximum(
                            acc[1 - d, r0:r1, c0:c1]
                            + rbuf[1, d, r0:r1, c0:c1].astype(jnp.float32), 0.0)
                        sbuf[2, d, r0:r1, c0:c1] = y.astype(jnp.bfloat16)
                        rdma(2, c, d).start()
                        out_ref[pl.ds(row0(slot) + r0, r1 - r0), c0:c1] = y

            for c, w in enumerate(p3):
                r0, r1, c0, c1 = w
                for d, slot in ((0, 2), (1, 1)):
                    with scope(f"p4w_{c}_{d}"):
                        recv(2, d, w)
                    with scope(f"p4_{c}_{d}"):
                        out_ref[pl.ds(row0(slot) + r0, r1 - r0), c0:c1] = (
                            rbuf[2, d, r0:r1, c0:c1].astype(jnp.float32))

            with scope("drain"):
                for phase in range(3):
                    for c in range(n_chunks[phase]):
                        for d in range(2):
                            rdma(phase, c, d).wait_send()

        pl.run_scoped(
            run,
            pltpu.SemaphoreType.DMA((len(loads),)),
            pltpu.SemaphoreType.DMA((n_rdma,)),
            pltpu.SemaphoreType.DMA((n_rdma,)),
        )

    return pl.pallas_call(
        body,
        out_shape=pltpu.VMEM((m, n), jnp.float32),
        in_specs=[pl.BlockSpec(memory_space=pl.ANY)] * 2,
        out_specs=pl.BlockSpec(memory_space=pltpu.VMEM),
        scratch_shapes=[
            pltpu.VMEM((N_DEV, G, k), jnp.float32),
            pltpu.VMEM((k, n), jnp.float32),
            pltpu.VMEM((N_DEV, G, k), jnp.bfloat16),
            pltpu.VMEM((k, n), jnp.bfloat16),
            pltpu.VMEM((3, 2, G, n), jnp.bfloat16),
            pltpu.VMEM((3, 2, G, n), jnp.bfloat16),
            pltpu.VMEM((2, G, n), jnp.float32),
        ],
        compiler_params=pltpu.CompilerParams(
            collective_id=0, vmem_limit_bytes=40 * 1024 * 1024),
    )


def pallas_dist_matmul_relu_kshard_i_m1024_n1024_k512_kernel(
    A: jax.Array,
    B: jax.Array,
):
    m, k = A.shape
    _, n = B.shape
    return _build(CFG, m, k, n)(A, B)
```

```python
import contextlib

import jax
import jax.numpy as jnp
from jax import lax
from jax.experimental import pallas as pl
from jax.experimental.pallas import tpu as pltpu

N_DEV = 4
G = 256
PAY = 120
LANE = 128


def _a_tiles(cfg, dev):
    tiles = list(cfg["a_ramp"])
    for (c0, c1), s in zip(cfg["a_cols"], cfg["a_splits"][dev]):
        tiles.append((c0, c1, [(0, s, 0), (s, G, 1)]))
    return tiles


_H = G // 2
CFG = dict(
    loads=[
        ("B", 0, 128), ("A", 2, 64, 192), ("A", 2, 32, 64), ("A", 2, 192, 224),
        ("B", 128, 256), ("A", 2, 0, 32), ("A", 2, 224, 256),
        ("B", 256, 384), ("B", 384, 512), ("A", 1, _H, G), ("A", 3, 0, _H),
        ("B", 512, 768), ("B", 768, 1024),
        ("A", 1, 0, _H), ("A", 3, _H, G), ("A", 0, 0, G),
    ],
    a_ramp=[
        (0, 128, [(64, 128, 0), (128, 192, 1)]),
        (0, 128, [(32, 64, 0), (192, 224, 1)]),
        (128, 256, [(32, 128, 0), (128, 224, 1)]),
        (0, 256, [(0, 32, 0), (224, 256, 1)]),
    ],
    a_cols=[(256, 384), (384, 512), (512, 768), (768, 896), (896, 1024)],
    a_splits=[(128, 128, 128, 128, 128), (128, 128, 160, 192, 176),
              (128, 128, 128, 128, 128), (128, 128, 96, 64, 80)],
    b_chunks=[
        (0, 256, (_H, G), (0, _H)), (256, 512, (_H, G), (0, _H)),
        (0, 256, (0, _H), (_H, G)), (256, 512, (0, _H), (_H, G)),
        (512, 768, (0, G), (0, G)), (768, 1024, (0, G), (0, G)),
    ],
    order=["A0", "A1", "A2", "A3", "A4", "A5", "B0", "B1", "A6", "A7", "A8",
           "B2", "B3", "B4", "B5"],
    d_chunks=[(0, 256), (256, 512), (512, 768), (768, 896), (896, 1024)],
    e_splits=[(56, 64, 64, 56, 56), (56, 48, 48, 64, 64),
              (56, 64, 64, 56, 56), (64, 72, 72, 56, 56)],
    scopes=False,
)


def _overlaps(w, v):
    return w[0] < v[1] and v[0] < w[1] and w[2] < v[3] and v[2] < w[3]


def _plan(cfg):
    xfers = {}

    def add(key, kind, d, wins):
        xfers[key] = (kind, d, wins, len(xfers))

    tiles = [_a_tiles(cfg, dev) for dev in range(N_DEV)]
    for t, (c0, c1, segs) in enumerate(tiles[0]):
        for i, (_, _, d) in enumerate(segs):
            add(("A", t, i), "A", d,
                [tiles[dev][t][2][i][:2] + (c0, c1) for dev in range(N_DEV)])
    for c, (c0, c1, *rows) in enumerate(cfg["b_chunks"]):
        for d in range(2):
            add(("B", c, d), "B", d, [rows[d] + (c0, c1)] * N_DEV)
    for c, (c0, c1) in enumerate(cfg["d_chunks"]):
        for d in range(2):
            add(("D", c, d), "D", d, [(0, PAY, c0, c1)] * N_DEV)
    for c, (c0, c1) in enumerate(cfg["d_chunks"]):
        for d in range(2):
            wins = []
            for dev in range(N_DEV):
                t = cfg["e_splits"][(dev + (-1 if d == 0 else 1)) % N_DEV][c]
                wins.append(((0, t) if d == 0 else (t, PAY)) + (c0, c1))
            add(("E", c, d), "E", d, wins)
    return xfers


def _pack(y):
    bits = lax.bitcast_convert_type(
        y.astype(jnp.bfloat16).astype(jnp.float32), jnp.int32)
    h = G // 2
    w = (bits[:h] & 0x7FFF0000) | (lax.shift_right_logical(bits[h:], 16) & 0x7FFF)
    extra = w[PAY:]
    spare = jnp.int32(-0x7FFF8000)
    return jnp.concatenate(
        [w[8 * j:8 * j + 8] | (lax.shift_left(extra, 15 - j) & spare)
         for j in range(15)], axis=0)


def _unpack(w):
    spare = jnp.int32(-0x7FFF8000)
    extra = None
    for j in range(15):
        b = lax.shift_right_logical(w[8 * j:8 * j + 8] & spare, 15 - j)
        extra = b if extra is None else extra | b
    w = jnp.concatenate([w, extra], axis=0)
    top = lax.bitcast_convert_type(w & 0x7FFF0000, jnp.float32)
    bot = lax.bitcast_convert_type(lax.shift_left(w, 16) & 0x7FFF0000, jnp.float32)
    return top, bot


def _build(cfg, m, k, n):
    xfers = _plan(cfg)
    loads, b_chunks, d_chunks = cfg["loads"], cfg["b_chunks"], cfg["d_chunks"]
    bf16, f32 = jnp.bfloat16, jnp.float32

    def scope(name):
        return jax.named_scope(name) if cfg["scopes"] else contextlib.nullcontext()

    def body(a_hbm, b_hbm, out_ref, a32, b32, a16, b16, s_a, r_a, s_b, r_b, pay):
        me = lax.axis_index("i")
        nbr = (lax.rem(me + 1, N_DEV), lax.rem(me + N_DEV - 1, N_DEV))

        def row0(slot):
            return pl.multiple_of(lax.rem(me + slot, N_DEV) * G, G)

        def run(load_sems, send_sems, recv_sems):
            load_cps = []
            for i, ld in enumerate(loads):
                if ld[0] == "B":
                    cols = pl.ds(ld[1], ld[2] - ld[1])
                    cp = pltpu.make_async_copy(
                        b_hbm.at[:, cols], b32.at[:, cols], load_sems.at[i])
                else:
                    _, s, r0, r1 = ld
                    cp = pltpu.make_async_copy(
                        a_hbm.at[pl.ds(row0(s) + r0, r1 - r0), :],
                        a32.at[s, pl.ds(r0, r1 - r0), :], load_sems.at[i])
                cp.start()
                load_cps.append(cp)

            barrier = pltpu.get_barrier_semaphore()
            for d in range(2):
                pl.semaphore_signal(
                    barrier, inc=1, device_id=(nbr[d],),
                    device_id_type=pl.DeviceIdType.MESH)

            loaded = [False] * len(loads)

            def need(slot, r0, r1, c0, c1):
                for i, ld in enumerate(loads):
                    if loaded[i]:
                        continue
                    if ld[0] == "B":
                        if not (ld[1] < c1 and c0 < ld[2]):
                            continue
                        load_cps[i].wait()
                        b16[:, ld[1]:ld[2]] = b32[:, ld[1]:ld[2]].astype(bf16)
                    else:
                        if not (ld[1] == slot and ld[2] < r1 and r0 < ld[3]):
                            continue
                        load_cps[i].wait()
                        a16[slot, ld[2]:ld[3], :] = (
                            a32[slot, ld[2]:ld[3], :].astype(bf16))
                    loaded[i] = True

            def rdma(key, window):
                kind, d, _, sem = xfers[key]
                r0, r1, c0, c1 = window
                win = (pl.ds(r0, r1 - r0), pl.ds(c0, c1 - c0))
                if kind == "A":
                    src, dst = s_a.at[win], r_a.at[(d,) + win]
                elif kind == "B":
                    src, dst = s_b.at[(d,) + win], r_b.at[(d,) + win]
                elif kind == "D":
                    src, dst = pay.at[(0,) + win], pay.at[((3, 1)[d],) + win]
                else:
                    src, dst = pay.at[((3, 1)[d],) + win], pay.at[(2,) + win]
                return pltpu.make_async_remote_copy(
                    src_ref=src, dst_ref=dst,
                    send_sem=send_sems.at[sem], recv_sem=recv_sems.at[sem],
                    device_id=(nbr[d],), device_id_type=pl.DeviceIdType.MESH)

            def for_sender(key, sender, fn):
                wins = xfers[key][2]
                if len(set(wins)) == 1:
                    fn(rdma(key, wins[0]))
                    return
                for w in sorted(set(wins)):
                    if w[1] == w[0]:
                        continue
                    devs = [dev for dev in range(N_DEV) if wins[dev] == w]
                    cond = sender == devs[0]
                    for dev in devs[1:]:
                        cond = cond | (sender == dev)
                    pl.when(cond)(lambda w=w: fn(rdma(key, w)))

            started, arrived = [], set()

            def send(key):
                for_sender(key, me, lambda cp: cp.start())
                started.append(key)

            def drain():
                while started:
                    for_sender(started.pop(0), me, lambda cp: cp.wait_send())

            def incoming(kind, d, w):
                return [key for key, t in xfers.items()
                        if t[0] == kind and t[1] == d
                        and any(_overlaps(w, v) for v in t[2])]

            def recv(kind, d, w):
                for key in incoming(kind, d, w):
                    if key not in arrived:
                        for_sender(key, nbr[1 - d], lambda cp: cp.wait_recv())
                        arrived.add(key)

            def matmul(segs, c0, c1):
                parts = [a16[s, r0:r1, :] for s, r0, r1 in segs]
                lhs = parts[0] if len(parts) == 1 else jnp.concatenate(parts, axis=0)
                return jnp.dot(lhs, b16[:, c0:c1], preferred_element_type=f32)

            def phase_a(t):
                c0, c1, segs = _a_tiles(cfg, 0)[t]
                with scope(f"Aw{t}"):
                    for r0, r1, _ in segs:
                        need(2, r0, r1, c0, c1)
                with scope(f"A{t}"):
                    if segs[0][1] == segs[1][0]:
                        rows = [(2, segs[0][0], segs[1][1])]
                    else:
                        rows = [(2, r0, r1) for r0, r1, _ in segs]
                    res = matmul(rows, c0, c1).astype(bf16)
                    o = 0
                    for _, r0, r1 in rows:
                        s_a[r0:r1, c0:c1] = res[o:o + r1 - r0]
                        o += r1 - r0
                if t == 0:
                    with scope("barrier"):
                        pl.semaphore_wait(barrier, 2)
                for i in range(len(segs)):
                    send(("A", t, i))

            def phase_b(c):
                c0, c1, *rows = b_chunks[c]
                with scope(f"Bw{c}"):
                    for d in range(2):
                        need((1, 3)[d], *rows[d], c0, c1)
                        recv("A", d, rows[d] + (c0, c1))
                with scope(f"B{c}"):
                    res = matmul([(1,) + rows[0], (3,) + rows[1]], c0, c1)
                    for d in range(2):
                        w0, w1 = rows[d]
                        base = (0, rows[0][1] - rows[0][0])[d] - w0
                        for j0 in range(c0, c1, LANE):
                            j1 = j0 + LANE
                            wins = [xfers[key][2]
                                    for key in incoming("A", d, (0, G, j0, j1))]
                            if d == 0:
                                split = [max(w[dev][1] for w in wins)
                                         for dev in range(N_DEV)]
                            else:
                                split = [min(w[dev][0] for w in wins)
                                         for dev in range(N_DEV)]
                            lo, hi = min(split), max(split)
                            spans = ((0, lo, "add" if d == 0 else "raw"),
                                     (lo, hi, "mix"),
                                     (hi, G, "raw" if d == 0 else "add"))
                            for r0, r1, how in spans:
                                r0, r1 = max(r0, w0), min(r1, w1)
                                if r1 <= r0:
                                    continue
                                v = res[base + r0:base + r1, j0 - c0:j1 - c0]
                                if how != "raw":
                                    x = r_a[d, r0:r1, j0:j1].astype(f32)
                                    if how == "mix":
                                        sp = jnp.int32(split[0])
                                        for dev in range(1, N_DEV):
                                            sp = jnp.where(
                                                nbr[1 - d] == dev, split[dev], sp)
                                        row = r0 + lax.broadcasted_iota(
                                            jnp.int32, (r1 - r0, LANE), 0)
                                        got = (row < sp) if d == 0 else (row >= sp)
                                        x = jnp.where(got, x, 0.0)
                                    v = v + x
                                s_b[d, r0:r1, j0:j1] = v.astype(bf16)
                for d in range(2):
                    send(("B", c, d))

            for task in cfg["order"]:
                (phase_a if task[0] == "A" else phase_b)(int(task[1:]))

            for c, (c0, c1) in enumerate(d_chunks):
                with scope(f"Dw{c}"):
                    need(0, 0, G, c0, c1)
                    recv("B", 0, (0, G, c0, c1))
                    recv("B", 1, (0, G, c0, c1))
                with scope(f"D{c}"):
                    y = (matmul([(0, 0, G)], c0, c1)
                         + r_b[0, :, c0:c1].astype(f32)
                         + r_b[1, :, c0:c1].astype(f32))
                    y = jnp.maximum(y, 0.0)
                    pay[0, :, c0:c1] = _pack(y)
                    for d in range(2):
                        send(("D", c, d))
                    out_ref[pl.ds(row0(0), G), c0:c1] = y

            def emit(slot, c0, c1):
                top, bot = _unpack(pay[slot, :, c0:c1])
                out_ref[pl.ds(row0(slot), G // 2), c0:c1] = top
                out_ref[pl.ds(row0(slot) + G // 2, G // 2), c0:c1] = bot

            for c, (c0, c1) in enumerate(d_chunks):
                for d in range(2):
                    with scope(f"Ew{c}_{d}"):
                        recv("D", d, (0, PAY, c0, c1))
                    with scope(f"E{c}_{d}"):
                        send(("E", c, d))
                        emit((3, 1)[d], c0, c1)

            last = started[-2:]
            del started[-2:]
            for c, (c0, c1) in enumerate(d_chunks):
                if c == len(d_chunks) - 1:
                    with scope("drain0"):
                        drain()
                with scope(f"Fw{c}"):
                    recv("E", 0, (0, PAY, c0, c1))
                    recv("E", 1, (0, PAY, c0, c1))
                with scope(f"F{c}"):
                    emit(2, c0, c1)
            started.extend(last)
            with scope("drain"):
                drain()

        pl.run_scoped(
            run,
            pltpu.SemaphoreType.DMA((len(loads),)),
            pltpu.SemaphoreType.DMA((len(xfers),)),
            pltpu.SemaphoreType.DMA((len(xfers),)),
        )

    return pl.pallas_call(
        body,
        out_shape=pltpu.VMEM((m, n), f32),
        in_specs=[pl.BlockSpec(memory_space=pl.ANY)] * 2,
        out_specs=pl.BlockSpec(memory_space=pltpu.VMEM),
        scratch_shapes=[
            pltpu.VMEM((N_DEV, G, k), f32),
            pltpu.VMEM((k, n), f32),
            pltpu.VMEM((N_DEV, G, k), bf16),
            pltpu.VMEM((k, n), bf16),
            pltpu.VMEM((G, n), bf16),
            pltpu.VMEM((2, G, n), bf16),
            pltpu.VMEM((2, G, n), bf16),
            pltpu.VMEM((2, G, n), bf16),
            pltpu.VMEM((N_DEV, PAY, n), jnp.int32),
        ],
        compiler_params=pltpu.CompilerParams(
            collective_id=0, vmem_limit_bytes=40 * 1024 * 1024),
    )


def pallas_dist_matmul_relu_kshard_i_m1024_n1024_k512_kernel(
    A: jax.Array,
    B: jax.Array,
):
    m, k = A.shape
    _, n = B.shape
    return _build(CFG, m, k, n)(A, B)
```

```python
import contextlib

import jax
import jax.numpy as jnp
from jax import lax
from jax.experimental import pallas as pl
from jax.experimental.pallas import tpu as pltpu

N_DEV = 4
G = 256
H = G // 2
PAY = 120
LANE = 128

CFG = dict(
    loads=[
        ("B", 0, 128), ("A", 2, 64, 192), ("A", 2, 32, 64), ("A", 2, 192, 224),
        ("B", 128, 256), ("A", 2, 0, 32), ("A", 2, 224, 256),
        ("B", 256, 384), ("B", 384, 512), ("A", 1, H, G), ("A", 3, 0, H),
        ("B", 512, 768), ("B", 768, 1024),
        ("A", 1, 0, H), ("A", 3, H, G), ("A", 0, 0, G),
    ],
    a_ramp=[
        (0, 128, [(64, 128, 0), (128, 192, 1)]),
        (0, 128, [(32, 64, 0), (192, 224, 1)]),
        (128, 256, [(32, 128, 0), (128, 224, 1)]),
        (0, 256, [(0, 32, 0), (224, 256, 1)]),
    ],
    a_cols=[(256, 384), (384, 512), (512, 768), (768, 896), (896, 1024)],
    a_splits=[(128, 128, 128, 128, 128), (128, 128, 160, 192, 176),
              (128, 128, 128, 128, 128), (128, 128, 96, 80, 80)],
    b_chunks=[
        (0, 256, (H, G), (0, H)), (256, 512, (H, G), (0, H)),
        (0, 256, (0, H), (H, G)), (256, 512, (0, H), (H, G)),
        (512, 768, (0, G), (0, G)), (768, 1024, (0, G), (0, G)),
    ],
    order=["A0", "A1", "A2", "A3", "A4", "A5", "B0", "A6", "B1", "A7", "A8",
           "B2", "B3", "B4", "B5"],
    d_chunks=[(0, 256), (256, 512), (512, 768), (768, 896), (896, 1024)],
    e_splits=[(56, 64, 64, 56, 56), (56, 48, 48, 64, 64),
              (56, 64, 64, 56, 56), (64, 72, 72, 56, 56)],
    scopes=False,
)


def _a_tiles(cfg, dev):
    tiles = list(cfg["a_ramp"])
    for (c0, c1), s in zip(cfg["a_cols"], cfg["a_splits"][dev]):
        tiles.append((c0, c1, [(0, s, 0), (s, G, 1)]))
    return tiles


def _overlaps(w, v):
    return w[0] < v[1] and v[0] < w[1] and w[2] < v[3] and v[2] < w[3]


def _plan(cfg):
    xfers = {}

    def add(key, d, wins):
        xfers[key] = (key[0], d, wins, len(xfers))

    tiles = [_a_tiles(cfg, dev) for dev in range(N_DEV)]
    for t, (c0, c1, segs) in enumerate(tiles[0]):
        for i, (_, _, d) in enumerate(segs):
            add(("A", t, i), d,
                [tiles[dev][t][2][i][:2] + (c0, c1) for dev in range(N_DEV)])
    for c, (c0, c1, *rows) in enumerate(cfg["b_chunks"]):
        for d in range(2):
            add(("B", c, d), d, [rows[d] + (c0, c1)] * N_DEV)
    for c, (c0, c1) in enumerate(cfg["d_chunks"]):
        for d in range(2):
            add(("D", c, d), d, [(0, PAY, c0, c1)] * N_DEV)
    for c, (c0, c1) in enumerate(cfg["d_chunks"]):
        for d in range(2):
            wins = []
            for dev in range(N_DEV):
                t = cfg["e_splits"][(dev + (-1 if d == 0 else 1)) % N_DEV][c]
                wins.append(((0, t) if d == 0 else (t, PAY)) + (c0, c1))
            add(("E", c, d), d, wins)
    return xfers


_SPARE = -0x7FFF8000


def _pack(y):
    bits = lax.bitcast_convert_type(
        y.astype(jnp.bfloat16).astype(jnp.float32), jnp.int32)
    w = (bits[:H] & 0x7FFF0000) | (lax.shift_right_logical(bits[H:], 16) & 0x7FFF)
    extra = w[PAY:]
    return jnp.concatenate(
        [w[8 * j:8 * j + 8] | (lax.shift_left(extra, 15 - j) & _SPARE)
         for j in range(15)], axis=0)


def _unpack(w):
    extra = None
    for j in range(15):
        b = lax.shift_right_logical(w[8 * j:8 * j + 8] & _SPARE, 15 - j)
        extra = b if extra is None else extra | b
    w = jnp.concatenate([w, extra], axis=0)
    top = lax.bitcast_convert_type(w & 0x7FFF0000, jnp.float32)
    bot = lax.bitcast_convert_type(lax.shift_left(w, 16) & 0x7FFF0000, jnp.float32)
    return top, bot


def _build(cfg, m, k, n):
    xfers = _plan(cfg)
    loads, b_chunks, d_chunks = cfg["loads"], cfg["b_chunks"], cfg["d_chunks"]
    bf16, f32 = jnp.bfloat16, jnp.float32

    def scope(name):
        return jax.named_scope(name) if cfg["scopes"] else contextlib.nullcontext()

    def body(a_hbm, b_hbm, out_ref, a_v, b_v, s_a, r_a, s_b, r_b, pay):
        me = lax.axis_index("i")
        nbr = (lax.rem(me + 1, N_DEV), lax.rem(me + N_DEV - 1, N_DEV))

        def row0(slot):
            return pl.multiple_of(lax.rem(me + slot, N_DEV) * G, G)

        def run(load_sems, send_sems, recv_sems):
            barrier = pltpu.get_barrier_semaphore()
            load_cps = []
            for i, ld in enumerate(loads):
                if i == 2:
                    for d in range(2):
                        pl.semaphore_signal(
                            barrier, inc=1, device_id=(nbr[d],),
                            device_id_type=pl.DeviceIdType.MESH)
                if ld[0] == "B":
                    cols = pl.ds(ld[1], ld[2] - ld[1])
                    cp = pltpu.make_async_copy(
                        b_hbm.at[:, cols], b_v.at[:, cols], load_sems.at[i])
                else:
                    _, s, r0, r1 = ld
                    cp = pltpu.make_async_copy(
                        a_hbm.at[pl.ds(row0(s) + r0, r1 - r0), :],
                        a_v.at[s, pl.ds(r0, r1 - r0), :], load_sems.at[i])
                cp.start()
                load_cps.append(cp)

            loaded = [False] * len(loads)

            def need(slot, r0, r1, c0, c1):
                for i, ld in enumerate(loads):
                    if ld[0] == "B":
                        hit = ld[1] < c1 and c0 < ld[2]
                    else:
                        hit = ld[1] == slot and ld[2] < r1 and r0 < ld[3]
                    if hit and not loaded[i]:
                        load_cps[i].wait()
                        loaded[i] = True

            def rdma(key, window):
                kind, d, _, sem = xfers[key]
                r0, r1, c0, c1 = window
                win = (pl.ds(r0, r1 - r0), pl.ds(c0, c1 - c0))
                if kind == "A":
                    src, dst = s_a.at[win], r_a.at[(d,) + win]
                elif kind == "B":
                    src, dst = s_b.at[(d,) + win], r_b.at[(d,) + win]
                elif kind == "D":
                    src, dst = pay.at[(0,) + win], pay.at[((3, 1)[d],) + win]
                else:
                    src, dst = pay.at[((3, 1)[d],) + win], pay.at[(2,) + win]
                return pltpu.make_async_remote_copy(
                    src_ref=src, dst_ref=dst,
                    send_sem=send_sems.at[sem], recv_sem=recv_sems.at[sem],
                    device_id=(nbr[d],), device_id_type=pl.DeviceIdType.MESH)

            def for_sender(key, sender, fn):
                wins = xfers[key][2]
                if len(set(wins)) == 1:
                    fn(rdma(key, wins[0]))
                    return
                for w in sorted(set(wins)):
                    if w[1] == w[0]:
                        continue
                    devs = [dev for dev in range(N_DEV) if wins[dev] == w]
                    cond = sender == devs[0]
                    for dev in devs[1:]:
                        cond = cond | (sender == dev)
                    pl.when(cond)(lambda w=w: fn(rdma(key, w)))

            started, arrived = [], set()

            def send(key):
                for_sender(key, me, lambda cp: cp.start())
                started.append(key)

            def drain():
                while started:
                    for_sender(started.pop(0), me, lambda cp: cp.wait_send())

            def incoming(kind, d, w):
                return [key for key, t in xfers.items()
                        if t[0] == kind and t[1] == d
                        and any(_overlaps(w, v) for v in t[2])]

            def recv(kind, d, w):
                for key in incoming(kind, d, w):
                    if key not in arrived:
                        for_sender(key, nbr[1 - d], lambda cp: cp.wait_recv())
                        arrived.add(key)

            def matmul(segs, c0, c1):
                parts = [a_v[s, r0:r1, :].astype(bf16) for s, r0, r1 in segs]
                lhs = parts[0] if len(parts) == 1 else jnp.concatenate(parts, axis=0)
                return jnp.dot(lhs, b_v[:, c0:c1].astype(bf16),
                               preferred_element_type=f32)

            def phase_a(t):
                c0, c1, segs = _a_tiles(cfg, 0)[t]
                with scope(f"Aw{t}"):
                    for r0, r1, _ in segs:
                        need(2, r0, r1, c0, c1)
                with scope(f"A{t}"):
                    if segs[0][1] == segs[1][0]:
                        rows = [(2, segs[0][0], segs[1][1])]
                    else:
                        rows = [(2, r0, r1) for r0, r1, _ in segs]
                    res = matmul(rows, c0, c1).astype(bf16)
                    early = len(set(xfers[("A", t, 0)][2])) == 1
                    o = 0
                    for i, (r0, r1, _) in enumerate(segs):
                        s_a[r0:r1, c0:c1] = res[o:o + r1 - r0]
                        o += r1 - r0
                        if t == 0 and i == 0:
                            pl.semaphore_wait(barrier, 2)
                        if early:
                            send(("A", t, i))
                    if not early:
                        for i in range(len(segs)):
                            send(("A", t, i))

            def phase_b(c):
                c0, c1, *rows = b_chunks[c]
                with scope(f"Bw{c}"):
                    for d in range(2):
                        need((1, 3)[d], *rows[d], c0, c1)
                        recv("A", d, rows[d] + (c0, c1))
                with scope(f"B{c}"):
                    res = matmul([(1,) + rows[0], (3,) + rows[1]], c0, c1)
                    for d in range(2):
                        w0, w1 = rows[d]
                        base = (0, rows[0][1] - rows[0][0])[d] - w0
                        for j0 in range(c0, c1, LANE):
                            j1 = j0 + LANE
                            wins = [xfers[key][2]
                                    for key in incoming("A", d, (0, G, j0, j1))]
                            if d == 0:
                                split = [max(w[dev][1] for w in wins)
                                         for dev in range(N_DEV)]
                            else:
                                split = [min(w[dev][0] for w in wins)
                                         for dev in range(N_DEV)]
                            lo, hi = min(split), max(split)
                            spans = ((0, lo, "add" if d == 0 else "raw"),
                                     (lo, hi, "mix"),
                                     (hi, G, "raw" if d == 0 else "add"))
                            for r0, r1, how in spans:
                                r0, r1 = max(r0, w0), min(r1, w1)
                                if r1 <= r0:
                                    continue
                                v = res[base + r0:base + r1, j0 - c0:j1 - c0]
                                if how != "raw":
                                    x = r_a[d, r0:r1, j0:j1].astype(f32)
                                    if how == "mix":
                                        sp = jnp.int32(split[0])
                                        for dev in range(1, N_DEV):
                                            sp = jnp.where(
                                                nbr[1 - d] == dev, split[dev], sp)
                                        row = r0 + lax.broadcasted_iota(
                                            jnp.int32, (r1 - r0, LANE), 0)
                                        got = (row < sp) if d == 0 else (row >= sp)
                                        x = jnp.where(got, x, 0.0)
                                    v = v + x
                                s_b[d, r0:r1, j0:j1] = v.astype(bf16)
                        send(("B", c, d))

            for task in cfg["order"]:
                (phase_a if task[0] == "A" else phase_b)(int(task[1:]))

            for c, (c0, c1) in enumerate(d_chunks):
                with scope(f"Dw{c}"):
                    need(0, 0, G, c0, c1)
                    recv("B", 0, (0, G, c0, c1))
                    recv("B", 1, (0, G, c0, c1))
                with scope(f"D{c}"):
                    y = (matmul([(0, 0, G)], c0, c1)
                         + r_b[0, :, c0:c1].astype(f32)
                         + r_b[1, :, c0:c1].astype(f32))
                    y = jnp.maximum(y, 0.0)
                    pay[0, :, c0:c1] = _pack(y)
                    for d in range(2):
                        send(("D", c, d))
                    out_ref[pl.ds(row0(0), G), c0:c1] = y

            def emit(slot, c0, c1):
                top, bot = _unpack(pay[slot, :, c0:c1])
                out_ref[pl.ds(row0(slot), H), c0:c1] = top
                out_ref[pl.ds(row0(slot) + H, H), c0:c1] = bot

            for c, (c0, c1) in enumerate(d_chunks):
                for d in range(2):
                    with scope(f"Ew{c}_{d}"):
                        recv("D", d, (0, PAY, c0, c1))
                    with scope(f"E{c}_{d}"):
                        send(("E", c, d))
                        emit((3, 1)[d], c0, c1)

            last = started[-2:]
            del started[-2:]
            for c, (c0, c1) in enumerate(d_chunks):
                if c == len(d_chunks) - 1:
                    with scope("drain0"):
                        drain()
                with scope(f"Fw{c}"):
                    recv("E", 0, (0, PAY, c0, c1))
                    recv("E", 1, (0, PAY, c0, c1))
                with scope(f"F{c}"):
                    emit(2, c0, c1)
            started.extend(last)
            with scope("drain"):
                drain()
            assert all(loaded) and len(arrived) == len(xfers)

        pl.run_scoped(
            run,
            pltpu.SemaphoreType.DMA((len(loads),)),
            pltpu.SemaphoreType.DMA((len(xfers),)),
            pltpu.SemaphoreType.DMA((len(xfers),)),
        )

    return pl.pallas_call(
        body,
        out_shape=pltpu.VMEM((m, n), f32),
        in_specs=[pl.BlockSpec(memory_space=pl.ANY)] * 2,
        out_specs=pl.BlockSpec(memory_space=pltpu.VMEM),
        scratch_shapes=[
            pltpu.VMEM((N_DEV, G, k), f32),
            pltpu.VMEM((k, n), f32),
            pltpu.VMEM((G, n), bf16),
            pltpu.VMEM((2, G, n), bf16),
            pltpu.VMEM((2, G, n), bf16),
            pltpu.VMEM((2, G, n), bf16),
            pltpu.VMEM((N_DEV, PAY, n), jnp.int32),
        ],
        compiler_params=pltpu.CompilerParams(
            collective_id=0, vmem_limit_bytes=32 * 1024 * 1024),
    )


def pallas_dist_matmul_relu_kshard_i_m1024_n1024_k512_kernel(
    A: jax.Array,
    B: jax.Array,
):
    m, k = A.shape
    _, n = B.shape
    return _build(CFG, m, k, n)(A, B)
```

```python
import contextlib

import jax
import jax.numpy as jnp
from jax import lax
from jax.experimental import pallas as pl
from jax.experimental.pallas import tpu as pltpu

N_DEV = 4
G = 256
H = G // 2
PAY = 120
LANE = 128
ALL, EVEN = (0, 1, 2, 3), (0, 2)


def _ramp(c0, c1, right, left):
    return (0, c0, c1, [(right, left)] * N_DEV)


def _full(st, c0, c1, splits):
    return (st, c0, c1,
            [None if s is None else ((0, s), (s, G)) for s in splits])


CFG = dict(
    loads=[
        ("B", 0, 128), ("A", 2, 64, 192), ("A", 2, 32, 64), ("A", 2, 192, 224),
        ("B", 128, 256), ("A", 2, 0, 32), ("A", 2, 224, 256),
        ("B", 256, 384), ("B", 384, 512), ("A", 1, H, G), ("A", 3, 0, H),
        ("B", 512, 768), ("A", 1, 0, H), ("B", 768, 1024),
        ("A", 3, H, G), ("A", 0, 0, G),
    ],
    a_tiles=[
        _ramp(0, 128, (64, 128), (128, 192)),
        _ramp(0, 128, (32, 64), (192, 224)),
        _ramp(128, 256, (32, 128), (128, 224)),
        _ramp(0, 256, (0, 32), (224, 256)),
        _full(0, 256, 384, [128] * 4),
        _full(0, 384, 512, [128] * 4),
        _full(0, 512, 640, [None, 144, None, 128]),
        _full(0, 640, 768, [None, 128, None, 128]),
        _full(1, 512, 768, [None, 144, None, 112]),
        _full(0, 768, 1024, [None, 160, None, 96]),
        _full(1, 768, 1024, [None, 160, None, 96]),
    ],
    b_chunks=[
        (0, 0, 256, (H, G), (0, H), ALL), (0, 256, 512, (H, G), (0, H), ALL),
        (0, 0, 256, (0, H), (H, G), ALL), (0, 256, 512, (0, H), (H, G), ALL),
        (0, 512, 640, (0, G), (0, G), EVEN), (0, 640, 768, (0, G), (0, G), EVEN),
        (1, 512, 768, (0, G), (0, G), EVEN),
        (0, 768, 1024, (0, G), (0, G), EVEN), (1, 768, 1024, (0, G), (0, G), EVEN),
    ],
    d_chunks=[
        (0, 0, 256, [56, 56, 56, 64]), (0, 256, 384, [64, 48, 64, 72]),
        (0, 384, 512, [64, 56, 64, 64]),
        (0, 512, 768, [None, 56, None, 64]), (1, 512, 768, [None, 56, None, 64]),
        (0, 768, 1024, [None, 120, None, 120]), (1, 768, 1024, [None, 0, None, 0]),
    ],
    order=["A0", "A1", "A2", "A3", "A4", "A5", "B0", "A6", "A7", "A8", "A9", "A10",
           "B1", "B2", "B3", "B4", "B5", "B6", "B7", "B8",
           "D0", "D1", "D2", "D3", "D4", "D5:0", "D6", "S5:1",
           "R0", "R1", "r2", "R3", "R4", "R5:0", "R6:1", "E2", "R6:0", "R5:1",
           "F0", "F1", "F3", "F4", "F5", "F6", "W2", "F2"],
    scopes=False,
)


def _overlaps(w, v):
    return w[0] < v[1] and v[0] < w[1] and w[2] < v[3] and v[2] < w[3]


def _dst(dev, d):
    return (dev + (1 if d == 0 else -1)) % N_DEV


def _plan(cfg):
    xfers = {}

    def add(key, st, wins):
        wins = [None if w is None or w[1] == w[0] else w for w in wins]
        xfers[key] = (st, wins, len(xfers))

    for t, (st, c0, c1, rows) in enumerate(cfg["a_tiles"]):
        for d in range(2):
            add(("A", t, d), st,
                [None if r is None else r[d] + (c0, c1) for r in rows])
    for c, (st, c0, c1, *rows, who) in enumerate(cfg["b_chunks"]):
        for d in range(2):
            add(("B", c, d), st, [rows[d] + (c0, c1) if dev in who else None
                                  for dev in range(N_DEV)])
    for c, (st, c0, c1, ts) in enumerate(cfg["d_chunks"]):
        for d in range(2):
            add(("D", c, d), st,
                [None if t is None else (0, PAY, c0, c1) for t in ts])
    for c, (st, c0, c1, ts) in enumerate(cfg["d_chunks"]):
        for d in range(2):
            wins = []
            for dev in range(N_DEV):
                t = ts[_dst(dev, 1 - d)]
                wins.append(None if t is None else
                            ((0, t) if d == 0 else (t, PAY)) + (c0, c1))
            add(("E", c, d), st, wins)
    return xfers


_SPARE = -0x7FFF8000


def _pack(y):
    bits = lax.bitcast_convert_type(
        y.astype(jnp.bfloat16).astype(jnp.float32), jnp.int32)
    w = (bits[:H] & 0x7FFF0000) | (lax.shift_right_logical(bits[H:], 16) & 0x7FFF)
    extra = w[PAY:]
    return jnp.concatenate(
        [w[8 * j:8 * j + 8] | (lax.shift_left(extra, 15 - j) & _SPARE)
         for j in range(15)], axis=0)


def _unpack(w):
    extra = None
    for j in range(15):
        b = lax.shift_right_logical(w[8 * j:8 * j + 8] & _SPARE, 15 - j)
        extra = b if extra is None else extra | b
    w = jnp.concatenate([w, extra], axis=0)
    top = lax.bitcast_convert_type(w & 0x7FFF0000, jnp.float32)
    bot = lax.bitcast_convert_type(lax.shift_left(w, 16) & 0x7FFF0000, jnp.float32)
    return top, bot


def _build(cfg, m, k, n):
    xfers = _plan(cfg)
    loads = cfg["loads"]
    a_tiles, b_chunks, d_chunks = cfg["a_tiles"], cfg["b_chunks"], cfg["d_chunks"]
    bf16, f32 = jnp.bfloat16, jnp.float32

    def scope(name):
        return jax.named_scope(name) if cfg["scopes"] else contextlib.nullcontext()

    def body(a_hbm, b_hbm, out_ref, a_v, b_v, s_a, r_a, s_b, r_b, pay):
        me = lax.axis_index("i")
        nbr = (lax.rem(me + 1, N_DEV), lax.rem(me + N_DEV - 1, N_DEV))

        def row0(slot):
            return pl.multiple_of(lax.rem(me + slot % N_DEV, N_DEV) * G, G)

        def run(load_sems, send_sems, recv_sems):
            barrier = pltpu.get_barrier_semaphore()
            load_cps = []
            for i, ld in enumerate(loads):
                if i == 2:
                    for d in range(2):
                        pl.semaphore_signal(
                            barrier, inc=1, device_id=(nbr[d],),
                            device_id_type=pl.DeviceIdType.MESH)
                if ld[0] == "B":
                    cols = pl.ds(ld[1], ld[2] - ld[1])
                    cp = pltpu.make_async_copy(
                        b_hbm.at[:, cols], b_v.at[:, cols], load_sems.at[i])
                else:
                    _, s, r0, r1 = ld
                    cp = pltpu.make_async_copy(
                        a_hbm.at[pl.ds(row0(s) + r0, r1 - r0), :],
                        a_v.at[s, pl.ds(r0, r1 - r0), :], load_sems.at[i])
                cp.start()
                load_cps.append(cp)

            ctx = [ALL]
            done = set()

            def on(devs, fn):
                devs = tuple(dev for dev in ctx[-1] if dev in devs)
                if not devs:
                    return
                if devs == ctx[-1]:
                    fn()
                    return
                cond = me == devs[0]
                for dev in devs[1:]:
                    cond = cond | (me == dev)

                def branch():
                    ctx.append(devs)
                    fn()
                    ctx.pop()
                pl.when(cond)(branch)

            def once(what, devs, fn):
                devs = [dev for dev in ctx[-1]
                        if dev in devs and (what, dev) not in done]
                done.update((what, dev) for dev in devs)
                on(devs, fn)

            def need(slot, r0, r1, c0, c1):
                for i, ld in enumerate(loads):
                    if ld[0] == "B":
                        hit = ld[1] < c1 and c0 < ld[2]
                    else:
                        hit = ld[1] == slot % N_DEV and ld[2] < r1 and r0 < ld[3]
                    if hit:
                        once(("load", i), ALL, load_cps[i].wait)

            def rdma(key, window):
                kind, _, d = key
                st, _, sem = xfers[key]
                r0, r1, c0, c1 = window
                win = (pl.ds(r0, r1 - r0), pl.ds(c0, c1 - c0))
                if kind == "A":
                    src, dst = s_a.at[(st,) + win], r_a.at[(st, d) + win]
                elif kind == "B":
                    src, dst = s_b.at[(st, d) + win], r_b.at[(st, d) + win]
                elif kind == "D":
                    src, dst = pay.at[(st, 0) + win], pay.at[(st, (3, 1)[d]) + win]
                else:
                    src, dst = pay.at[(st, (3, 1)[d]) + win], pay.at[(st, 2) + win]
                return pltpu.make_async_remote_copy(
                    src_ref=src, dst_ref=dst,
                    send_sem=send_sems.at[sem], recv_sem=recv_sems.at[sem],
                    device_id=(nbr[d],), device_id_type=pl.DeviceIdType.MESH)

            def each_window(what, key, shift, fn):
                wins = xfers[key][1]
                for w in sorted(set(w for w in wins if w is not None)):
                    devs = [(dev + shift) % N_DEV
                            for dev in range(N_DEV) if wins[dev] == w]
                    once((what, key), devs, lambda w=w: fn(rdma(key, w)))

            started = []

            def send(key):
                each_window("start", key, 0, lambda cp: cp.start())
                started.append(key)

            def drain(keep=()):
                for key in started:
                    if key not in keep:
                        each_window("sent", key, 0, lambda cp: cp.wait_send())

            def incoming(kind, st, d, w):
                return [key for key, t in xfers.items()
                        if key[0] == kind and key[2] == d and t[0] == st
                        and any(v is not None and _overlaps(w, v) for v in t[1])]

            def recv(kind, st, d, w):
                for key in incoming(kind, st, d, w):
                    each_window("recv", key, 1 if d == 0 else -1,
                                lambda cp: cp.wait_recv())

            def matmul(segs, c0, c1):
                parts = [a_v[s % N_DEV, r0:r1, :].astype(bf16) for s, r0, r1 in segs]
                lhs = parts[0] if len(parts) == 1 else jnp.concatenate(parts, axis=0)
                return jnp.dot(lhs, b_v[:, c0:c1].astype(bf16),
                               preferred_element_type=f32)

            def phase_a(t):
                st, c0, c1, rows = a_tiles[t]
                who = [dev for dev in range(N_DEV) if rows[dev] is not None]
                segs = rows[who[0]]
                early = len(set(rows[dev] for dev in who)) == 1

                def go():
                    with scope(f"Aw{t}"):
                        for r0, r1 in segs:
                            need(2 - st, r0, r1, c0, c1)
                    with scope(f"A{t}"):
                        if segs[0][1] == segs[1][0]:
                            lhs = [(2 - st, segs[0][0], segs[1][1])]
                        else:
                            lhs = [(2 - st,) + seg for seg in segs]
                        res = matmul(lhs, c0, c1).astype(bf16)
                        o = 0
                        for d, (r0, r1) in enumerate(segs):
                            s_a[st, r0:r1, c0:c1] = res[o:o + r1 - r0]
                            o += r1 - r0
                            if t == 0 and d == 0:
                                pl.semaphore_wait(barrier, 2)
                            if early:
                                send(("A", t, d))
                        if not early:
                            for d in range(2):
                                send(("A", t, d))
                on(who, go)

            def phase_b(c):
                st, c0, c1, *rows, who = b_chunks[c]

                def block(res, d, j0):
                    w0, w1 = rows[d]
                    base = (0, rows[0][1] - rows[0][0])[d] - w0
                    j1 = j0 + LANE
                    wins = [xfers[key][1]
                            for key in incoming("A", st, d, (0, G, j0, j1))]
                    split = {}
                    for dev in who:
                        src = _dst(dev, 1 - d)
                        split[dev] = (max(w[src][1] for w in wins) if d == 0
                                      else min(w[src][0] for w in wins))
                    lo, hi = min(split.values()), max(split.values())
                    spans = ((0, lo, "add" if d == 0 else "raw"),
                             (lo, hi, "mix"),
                             (hi, G, "raw" if d == 0 else "add"))
                    for r0, r1, how in spans:
                        r0, r1 = max(r0, w0), min(r1, w1)
                        if r1 <= r0:
                            continue
                        v = res[base + r0:base + r1, j0 - c0:j1 - c0]
                        if how != "raw":
                            x = r_a[st, d, r0:r1, j0:j1].astype(f32)
                            if how == "mix":
                                sp = jnp.int32(split[who[0]])
                                for dev in who[1:]:
                                    sp = jnp.where(me == dev, split[dev], sp)
                                row = r0 + lax.broadcasted_iota(
                                    jnp.int32, (r1 - r0, LANE), 0)
                                got = (row < sp) if d == 0 else (row >= sp)
                                x = jnp.where(got, x, 0.0)
                            v = v + x
                        s_b[st, d, r0:r1, j0:j1] = v.astype(bf16)

                def go():
                    with scope(f"Bw{c}"):
                        for d in range(2):
                            need((1, 3)[d] - st, *rows[d], c0, c1)
                            recv("A", st, d, rows[d] + (c0, c1))
                    with scope(f"B{c}"):
                        res = matmul(
                            [(1 - st,) + rows[0], (3 - st,) + rows[1]], c0, c1)
                        for d in range(2):
                            for j0 in range(c0, c1, LANE):
                                block(res, d, j0)
                            send(("B", c, d))
                on(who, go)

            def roots(c, shift):
                return [(dev + shift) % N_DEV for dev in range(N_DEV)
                        if d_chunks[c][3][dev] is not None]

            def phase_d(c, dirs=(0, 1)):
                st, c0, c1, _ = d_chunks[c]

                def go():
                    with scope(f"Dw{c}"):
                        need(-st, 0, G, c0, c1)
                        recv("B", st, 0, (0, G, c0, c1))
                        recv("B", st, 1, (0, G, c0, c1))
                    with scope(f"D{c}"):
                        y = (matmul([(-st, 0, G)], c0, c1)
                             + r_b[st, 0, :, c0:c1].astype(f32)
                             + r_b[st, 1, :, c0:c1].astype(f32))
                        y = jnp.maximum(y, 0.0)
                        pay[st, 0, :, c0:c1] = _pack(y)
                        for d in dirs:
                            send(("D", c, d))
                        out_ref[pl.ds(row0(-st), G), c0:c1] = y
                on(roots(c, 0), go)

            def emit(st, slot, c0, c1):
                top, bot = _unpack(pay[st, slot, :, c0:c1])
                out_ref[pl.ds(row0(slot - st), H), c0:c1] = top
                out_ref[pl.ds(row0(slot - st) + H, H), c0:c1] = bot

            def phase_r(c, dirs=(0, 1), forward=True):
                st, c0, c1, _ = d_chunks[c]

                def go():
                    for d in dirs:
                        with scope(f"Rw{c}_{d}"):
                            recv("D", st, d, (0, PAY, c0, c1))
                        with scope(f"R{c}_{d}"):
                            if forward:
                                send(("E", c, d))
                            emit(st, (3, 1)[d], c0, c1)
                on(roots(c, 1), go)

            def phase_e(c):
                for d in range(2):
                    send(("E", c, d))

            def phase_f(c):
                st, c0, c1, _ = d_chunks[c]

                def go():
                    with scope(f"Fw{c}"):
                        recv("E", st, 0, (0, PAY, c0, c1))
                        recv("E", st, 1, (0, PAY, c0, c1))
                    with scope(f"F{c}"):
                        emit(st, 2, c0, c1)
                on(roots(c, 2), go)

            tasks = dict(
                A=phase_a, B=phase_b, D=phase_d, R=phase_r, E=phase_e, F=phase_f,
                r=lambda c: phase_r(c, forward=False),
                S=lambda c, dirs: send(("D", c, dirs[0])),
                W=lambda c: drain([("E", c, 0), ("E", c, 1)]))
            for task in cfg["order"]:
                c, _, d = task[1:].partition(":")
                tasks[task[0]](int(c), *([(int(d),)] if d else []))
            with scope("drain"):
                drain()

            for i in range(len(loads)):
                assert all((("load", i), dev) in done for dev in ALL)
            for key, (_, wins, _) in xfers.items():
                for dev, w in enumerate(wins):
                    if w is not None:
                        assert (("start", key), dev) in done
                        assert (("sent", key), dev) in done
                        assert (("recv", key), _dst(dev, key[2])) in done

        pl.run_scoped(
            run,
            pltpu.SemaphoreType.DMA((len(loads),)),
            pltpu.SemaphoreType.DMA((len(xfers),)),
            pltpu.SemaphoreType.DMA((len(xfers),)),
        )

    return pl.pallas_call(
        body,
        out_shape=pltpu.VMEM((m, n), f32),
        in_specs=[pl.BlockSpec(memory_space=pl.ANY)] * 2,
        out_specs=pl.BlockSpec(memory_space=pltpu.VMEM),
        scratch_shapes=[
            pltpu.VMEM((N_DEV, G, k), f32),
            pltpu.VMEM((k, n), f32),
            pltpu.VMEM((2, G, n), bf16),
            pltpu.VMEM((2, 2, G, n), bf16),
            pltpu.VMEM((2, 2, G, n), bf16),
            pltpu.VMEM((2, 2, G, n), bf16),
            pltpu.VMEM((2, N_DEV, PAY, n), jnp.int32),
        ],
        compiler_params=pltpu.CompilerParams(
            collective_id=0, vmem_limit_bytes=40 * 1024 * 1024),
    )


def pallas_dist_matmul_relu_kshard_i_m1024_n1024_k512_kernel(
    A: jax.Array,
    B: jax.Array,
):
    m, k = A.shape
    _, n = B.shape
    return _build(CFG, m, k, n)(A, B)
```

```python
import contextlib

import jax
import jax.numpy as jnp
from jax import lax
from jax.experimental import pallas as pl
from jax.experimental.pallas import tpu as pltpu

N_DEV = 4
G = 256
H = G // 2
PAY = 120
LANE = 128
ALL, EVEN = (0, 1, 2, 3), (0, 2)


def _ramp(c0, c1, right, left):
    return (0, c0, c1, [(right, left)] * N_DEV)


def _full(st, c0, c1, splits):
    return (st, c0, c1,
            [None if s is None else ((0, s), (s, G)) for s in splits])


CFG = dict(
    loads=[
        ("B", 0, 128), ("A", 2, 64, 192), ("A", 2, 32, 64), ("A", 2, 192, 224),
        ("B", 128, 256), ("A", 2, 0, 32), ("A", 2, 224, 256),
        ("B", 256, 384), ("B", 384, 512), ("A", 1, H, G), ("A", 3, 0, H),
        ("B", 512, 768), ("A", 1, 0, H), ("B", 768, 1024),
        ("A", 3, H, G), ("A", 0, 0, G),
    ],
    a_tiles=[
        _ramp(0, 128, (64, 128), (128, 192)),
        _ramp(0, 128, (32, 64), (192, 224)),
        _ramp(128, 256, (32, 128), (128, 224)),
        _ramp(0, 256, (0, 32), (224, 256)),
        _full(0, 256, 384, [128] * 4),
        _full(0, 384, 512, [128] * 4),
        _full(0, 512, 640, [None, 144, None, 128]),
        _full(0, 640, 768, [None, 128, None, 128]),
        _full(1, 512, 768, [None, 144, None, 112]),
        _full(0, 768, 1024, [None, 160, None, 96]),
        _full(1, 768, 1024, [None, 160, None, 96]),
    ],
    b_chunks=[
        (0, 0, 256, (H, G), (0, H), ALL), (0, 256, 512, (H, G), (0, H), ALL),
        (0, 0, 256, (0, H), (H, G), ALL), (0, 256, 512, (0, H), (H, G), ALL),
        (0, 512, 640, (0, G), (0, G), EVEN), (0, 640, 768, (0, G), (0, G), EVEN),
        (1, 512, 768, (0, G), (0, G), EVEN),
        (0, 768, 1024, (0, G), (0, G), EVEN), (1, 768, 1024, (0, G), (0, G), EVEN),
    ],
    d_chunks=[
        (0, 0, 256, [56, 56, 56, 64]), (0, 256, 384, [64, 48, 64, 72]),
        (0, 384, 512, [64, 56, 64, 64]),
        (0, 512, 768, [None, 56, None, 64]), (1, 512, 768, [None, 56, None, 64]),
        (0, 768, 1024, [None, 120, None, 120]), (1, 768, 1024, [None, 0, None, 0]),
    ],
    order=["A0", "A1", "A2", "A3", "A4", "A5", "B0", "A6", "A7", "A8", "A9", "A10",
           "B1", "B2", "B3", "B4", "B5", "B6", "B7", "B8",
           "D0", "D1", "D2", "D3", "D4", "D5:0", "D6", "S5:1",
           "R0", "R1", "r2", "R3", "R4", "R5:0", "R6:1", "E2", "R6:0", "R5:1",
           "F0", "F1", "F3", "F4", "F5", "F6", "W2", "F2"],
    scopes=False,
)


def _overlaps(w, v):
    return w[0] < v[1] and v[0] < w[1] and w[2] < v[3] and v[2] < w[3]


def _dst(dev, d):
    return (dev + (1 if d == 0 else -1)) % N_DEV


def _plan(cfg):
    xfers = {}

    def add(key, st, wins):
        wins = [None if w is None or w[1] == w[0] else w for w in wins]
        xfers[key] = (st, wins, len(xfers))

    for t, (st, c0, c1, rows) in enumerate(cfg["a_tiles"]):
        for d in range(2):
            add(("A", t, d), st,
                [None if r is None else r[d] + (c0, c1) for r in rows])
    for c, (st, c0, c1, *rows, who) in enumerate(cfg["b_chunks"]):
        for d in range(2):
            add(("B", c, d), st, [rows[d] + (c0, c1) if dev in who else None
                                  for dev in range(N_DEV)])
    for c, (st, c0, c1, ts) in enumerate(cfg["d_chunks"]):
        for d in range(2):
            add(("D", c, d), st,
                [None if t is None else (0, PAY, c0, c1) for t in ts])
    for c, (st, c0, c1, ts) in enumerate(cfg["d_chunks"]):
        for d in range(2):
            wins = []
            for dev in range(N_DEV):
                t = ts[_dst(dev, 1 - d)]
                wins.append(None if t is None else
                            ((0, t) if d == 0 else (t, PAY)) + (c0, c1))
            add(("E", c, d), st, wins)
    return xfers


_SPARE = -0x7FFF8000


def _pack(y):
    bits = lax.bitcast_convert_type(
        y.astype(jnp.bfloat16).astype(jnp.float32), jnp.int32)
    w = (bits[:H] & 0x7FFF0000) | (lax.shift_right_logical(bits[H:], 16) & 0x7FFF)
    extra = w[PAY:]
    return jnp.concatenate(
        [w[8 * j:8 * j + 8] | (lax.shift_left(extra, 15 - j) & _SPARE)
         for j in range(15)], axis=0)


def _unpack(w):
    extra = None
    for j in range(15):
        b = lax.shift_right_logical(w[8 * j:8 * j + 8] & _SPARE, 15 - j)
        extra = b if extra is None else extra | b
    w = jnp.concatenate([w, extra], axis=0)
    top = lax.bitcast_convert_type(w & 0x7FFF0000, jnp.float32)
    bot = lax.bitcast_convert_type(lax.shift_left(w, 16) & 0x7FFF0000, jnp.float32)
    return top, bot


def _build(cfg, m, k, n):
    xfers = _plan(cfg)
    loads = cfg["loads"]
    a_tiles, b_chunks, d_chunks = cfg["a_tiles"], cfg["b_chunks"], cfg["d_chunks"]
    bf16, f32 = jnp.bfloat16, jnp.float32

    def scope(name):
        return jax.named_scope(name) if cfg["scopes"] else contextlib.nullcontext()

    def body(a_hbm, b_hbm, out_ref, a_v, b_v, s_a, r_a, s_b, r_b, pay):

        def run(load_sems, send_sems, recv_sems):
            def load_b(i):
                cols = pl.ds(loads[i][1], loads[i][2] - loads[i][1])
                return pltpu.make_async_copy(
                    b_hbm.at[:, cols], b_v.at[:, cols], load_sems.at[i])

            load_cps = [load_b(0)]
            load_cps[0].start()

            me = lax.axis_index("i")
            nbr = (lax.rem(me + 1, N_DEV), lax.rem(me + N_DEV - 1, N_DEV))

            def row0(slot):
                return pl.multiple_of(lax.rem(me + slot % N_DEV, N_DEV) * G, G)

            barrier = pltpu.get_barrier_semaphore()
            for d in range(2):
                pl.semaphore_signal(
                    barrier, inc=1, device_id=(nbr[d],),
                    device_id_type=pl.DeviceIdType.MESH)
            for i in range(1, len(loads)):
                if loads[i][0] == "B":
                    cp = load_b(i)
                else:
                    _, s, r0, r1 = loads[i]
                    cp = pltpu.make_async_copy(
                        a_hbm.at[pl.ds(row0(s) + r0, r1 - r0), :],
                        a_v.at[s, pl.ds(r0, r1 - r0), :], load_sems.at[i])
                cp.start()
                load_cps.append(cp)

            ctx = [ALL]
            done = set()

            def on(devs, fn):
                devs = tuple(dev for dev in ctx[-1] if dev in devs)
                if not devs:
                    return
                if devs == ctx[-1]:
                    fn()
                    return
                cond = me == devs[0]
                for dev in devs[1:]:
                    cond = cond | (me == dev)

                def branch():
                    ctx.append(devs)
                    fn()
                    ctx.pop()
                pl.when(cond)(branch)

            def once(what, devs, fn):
                devs = [dev for dev in ctx[-1]
                        if dev in devs and (what, dev) not in done]
                done.update((what, dev) for dev in devs)
                on(devs, fn)

            def need(slot, r0, r1, c0, c1):
                for i, ld in enumerate(loads):
                    if ld[0] == "B":
                        hit = ld[1] < c1 and c0 < ld[2]
                    else:
                        hit = ld[1] == slot % N_DEV and ld[2] < r1 and r0 < ld[3]
                    if hit:
                        once(("load", i), ALL, load_cps[i].wait)

            def rdma(key, window):
                kind, _, d = key
                st, _, sem = xfers[key]
                r0, r1, c0, c1 = window
                win = (pl.ds(r0, r1 - r0), pl.ds(c0, c1 - c0))
                if kind == "A":
                    src, dst = s_a.at[(st,) + win], r_a.at[(st, d) + win]
                elif kind == "B":
                    src, dst = s_b.at[(st, d) + win], r_b.at[(st, d) + win]
                elif kind == "D":
                    src, dst = pay.at[(st, 0) + win], pay.at[(st, (3, 1)[d]) + win]
                else:
                    src, dst = pay.at[(st, (3, 1)[d]) + win], pay.at[(st, 2) + win]
                return pltpu.make_async_remote_copy(
                    src_ref=src, dst_ref=dst,
                    send_sem=send_sems.at[sem], recv_sem=recv_sems.at[sem],
                    device_id=(nbr[d],), device_id_type=pl.DeviceIdType.MESH)

            def each_window(what, key, shift, fn):
                wins = xfers[key][1]
                for w in sorted(set(w for w in wins if w is not None)):
                    devs = [(dev + shift) % N_DEV
                            for dev in range(N_DEV) if wins[dev] == w]
                    once((what, key), devs, lambda w=w: fn(rdma(key, w)))

            started = []

            def send(key):
                each_window("start", key, 0, lambda cp: cp.start())
                started.append(key)

            def drain(keep=()):
                for key in started:
                    if key not in keep:
                        each_window("sent", key, 0, lambda cp: cp.wait_send())

            def incoming(kind, st, d, w):
                return [key for key, t in xfers.items()
                        if key[0] == kind and key[2] == d and t[0] == st
                        and any(v is not None and _overlaps(w, v) for v in t[1])]

            def recv(kind, st, d, w):
                for key in incoming(kind, st, d, w):
                    each_window("recv", key, 1 if d == 0 else -1,
                                lambda cp: cp.wait_recv())

            def matmul(segs, c0, c1):
                parts = [a_v[s % N_DEV, r0:r1, :].astype(bf16) for s, r0, r1 in segs]
                lhs = parts[0] if len(parts) == 1 else jnp.concatenate(parts, axis=0)
                return jnp.dot(lhs, b_v[:, c0:c1].astype(bf16),
                               preferred_element_type=f32)

            def phase_a(t):
                st, c0, c1, rows = a_tiles[t]
                who = [dev for dev in range(N_DEV) if rows[dev] is not None]
                segs = rows[who[0]]
                early = len(set(rows[dev] for dev in who)) == 1

                def go():
                    with scope(f"Aw{t}"):
                        for r0, r1 in segs:
                            need(2 - st, r0, r1, c0, c1)
                    with scope(f"A{t}"):
                        if segs[0][1] == segs[1][0]:
                            lhs = [(2 - st, segs[0][0], segs[1][1])]
                        else:
                            lhs = [(2 - st,) + seg for seg in segs]
                        res = matmul(lhs, c0, c1).astype(bf16)
                        o = 0
                        for d, (r0, r1) in enumerate(segs):
                            s_a[st, r0:r1, c0:c1] = res[o:o + r1 - r0]
                            o += r1 - r0
                            if t == 0 and d == 0:
                                pl.semaphore_wait(barrier, 2)
                            if early:
                                send(("A", t, d))
                        if not early:
                            for d in range(2):
                                send(("A", t, d))
                on(who, go)

            def phase_b(c):
                st, c0, c1, *rows, who = b_chunks[c]

                def block(res, d, j0):
                    w0, w1 = rows[d]
                    base = (0, rows[0][1] - rows[0][0])[d] - w0
                    j1 = j0 + LANE
                    wins = [xfers[key][1]
                            for key in incoming("A", st, d, (0, G, j0, j1))]
                    split = {}
                    for dev in who:
                        src = _dst(dev, 1 - d)
                        split[dev] = (max(w[src][1] for w in wins) if d == 0
                                      else min(w[src][0] for w in wins))
                    lo, hi = min(split.values()), max(split.values())
                    spans = ((0, lo, "add" if d == 0 else "raw"),
                             (lo, hi, "mix"),
                             (hi, G, "raw" if d == 0 else "add"))
                    for r0, r1, how in spans:
                        r0, r1 = max(r0, w0), min(r1, w1)
                        if r1 <= r0:
                            continue
                        v = res[base + r0:base + r1, j0 - c0:j1 - c0]
                        if how != "raw":
                            x = r_a[st, d, r0:r1, j0:j1].astype(f32)
                            if how == "mix":
                                sp = jnp.int32(split[who[0]])
                                for dev in who[1:]:
                                    sp = jnp.where(me == dev, split[dev], sp)
                                row = r0 + lax.broadcasted_iota(
                                    jnp.int32, (r1 - r0, LANE), 0)
                                got = (row < sp) if d == 0 else (row >= sp)
                                x = jnp.where(got, x, 0.0)
                            v = v + x
                        s_b[st, d, r0:r1, j0:j1] = v.astype(bf16)

                def go():
                    with scope(f"Bw{c}"):
                        for d in range(2):
                            need((1, 3)[d] - st, *rows[d], c0, c1)
                            recv("A", st, d, rows[d] + (c0, c1))
                    with scope(f"B{c}"):
                        res = matmul(
                            [(1 - st,) + rows[0], (3 - st,) + rows[1]], c0, c1)
                        for d in range(2):
                            for j0 in range(c0, c1, LANE):
                                block(res, d, j0)
                            send(("B", c, d))
                on(who, go)

            def roots(c, shift):
                return [(dev + shift) % N_DEV for dev in range(N_DEV)
                        if d_chunks[c][3][dev] is not None]

            def phase_d(c, dirs=(0, 1)):
                st, c0, c1, _ = d_chunks[c]

                def go():
                    with scope(f"Dw{c}"):
                        need(-st, 0, G, c0, c1)
                        recv("B", st, 0, (0, G, c0, c1))
                        recv("B", st, 1, (0, G, c0, c1))
                    with scope(f"D{c}"):
                        y = (matmul([(-st, 0, G)], c0, c1)
                             + r_b[st, 0, :, c0:c1].astype(f32)
                             + r_b[st, 1, :, c0:c1].astype(f32))
                        y = jnp.maximum(y, 0.0)
                        pay[st, 0, :, c0:c1] = _pack(y)
                        for d in dirs:
                            send(("D", c, d))
                        out_ref[pl.ds(row0(-st), G), c0:c1] = y
                on(roots(c, 0), go)

            def emit(st, slot, c0, c1):
                top, bot = _unpack(pay[st, slot, :, c0:c1])
                out_ref[pl.ds(row0(slot - st), H), c0:c1] = top
                out_ref[pl.ds(row0(slot - st) + H, H), c0:c1] = bot

            def phase_r(c, dirs=(0, 1), forward=True):
                st, c0, c1, _ = d_chunks[c]

                def go():
                    for d in dirs:
                        with scope(f"Rw{c}_{d}"):
                            recv("D", st, d, (0, PAY, c0, c1))
                        with scope(f"R{c}_{d}"):
                            if forward:
                                send(("E", c, d))
                            emit(st, (3, 1)[d], c0, c1)
                on(roots(c, 1), go)

            def phase_e(c):
                for d in range(2):
                    send(("E", c, d))

            def phase_f(c):
                st, c0, c1, _ = d_chunks[c]

                def go():
                    with scope(f"Fw{c}"):
                        recv("E", st, 0, (0, PAY, c0, c1))
                        recv("E", st, 1, (0, PAY, c0, c1))
                    with scope(f"F{c}"):
                        emit(st, 2, c0, c1)
                on(roots(c, 2), go)

            tasks = dict(
                A=phase_a, B=phase_b, D=phase_d, R=phase_r, E=phase_e, F=phase_f,
                r=lambda c: phase_r(c, forward=False),
                S=lambda c, dirs: send(("D", c, dirs[0])),
                W=lambda c: drain([("E", c, 0), ("E", c, 1)]))
            for task in cfg["order"]:
                c, _, d = task[1:].partition(":")
                tasks[task[0]](int(c), *([(int(d),)] if d else []))
            with scope("drain"):
                drain()

            for i in range(len(loads)):
                assert all((("load", i), dev) in done for dev in ALL)
            for key, (_, wins, _) in xfers.items():
                for dev, w in enumerate(wins):
                    if w is not None:
                        assert (("start", key), dev) in done
                        assert (("sent", key), dev) in done
                        assert (("recv", key), _dst(dev, key[2])) in done

        pl.run_scoped(
            run,
            pltpu.SemaphoreType.DMA((len(loads),)),
            pltpu.SemaphoreType.DMA((len(xfers),)),
            pltpu.SemaphoreType.DMA((len(xfers),)),
        )

    return pl.pallas_call(
        body,
        out_shape=pltpu.VMEM((m, n), f32),
        in_specs=[pl.BlockSpec(memory_space=pl.ANY)] * 2,
        out_specs=pl.BlockSpec(memory_space=pltpu.VMEM),
        scratch_shapes=[
            pltpu.VMEM((N_DEV, G, k), f32),
            pltpu.VMEM((k, n), f32),
            pltpu.VMEM((2, G, n), bf16),
            pltpu.VMEM((2, 2, G, n), bf16),
            pltpu.VMEM((2, 2, G, n), bf16),
            pltpu.VMEM((2, 2, G, n), bf16),
            pltpu.VMEM((2, N_DEV, PAY, n), jnp.int32),
        ],
        compiler_params=pltpu.CompilerParams(
            collective_id=0, vmem_limit_bytes=40 * 1024 * 1024),
    )


def pallas_dist_matmul_relu_kshard_i_m1024_n1024_k512_kernel(
    A: jax.Array,
    B: jax.Array,
):
    m, k = A.shape
    _, n = B.shape
    return _build(CFG, m, k, n)(A, B)
```
